```python
import numpy as np

kernel_name = "dist_sort_i_m128_n64"

def setup_inputs():
    return {"x": np.random.randn(512, 64).astype(np.float32)}

def reference(x: np.ndarray) -> np.ndarray:
    return np.sort(x, axis=0)
```

```python
import jax
import jax.numpy as jnp
from jax import lax
from jax.experimental import pallas as pl
from jax.experimental.pallas import tpu as pltpu

_ROWS, _COLS = 128, 64
_SPLIT = 32
_DIRECT = 24
_LOADED = _COLS - _DIRECT
_TILE = (8, 128)

_NETWORKS = {
    8: (
        ((0, 2), (1, 3), (4, 6), (5, 7)),
        ((0, 4), (1, 5), (2, 6), (3, 7)),
        ((0, 1), (2, 3), (4, 5), (6, 7)),
        ((2, 4), (3, 5)),
        ((1, 4), (3, 6)),
        ((1, 2), (3, 4), (5, 6)),
    ),
    16: (
        ((0, 13), (1, 12), (2, 15), (3, 14), (4, 8), (5, 6), (7, 11), (9, 10)),
        ((0, 5), (1, 7), (2, 9), (3, 4), (6, 13), (8, 14), (10, 15), (11, 12)),
        ((0, 1), (2, 3), (4, 5), (6, 8), (7, 9), (10, 11), (12, 13), (14, 15)),
        ((0, 2), (1, 3), (4, 10), (5, 11), (6, 7), (8, 9), (12, 14), (13, 15)),
        ((1, 2), (3, 12), (4, 6), (5, 7), (8, 10), (9, 11), (13, 14)),
        ((1, 4), (2, 6), (5, 8), (7, 10), (9, 13), (11, 14)),
        ((2, 4), (3, 6), (9, 12), (11, 13)),
        ((3, 5), (6, 8), (7, 9), (10, 12)),
        ((3, 4), (5, 6), (7, 8), (9, 10), (11, 12)),
        ((6, 7), (8, 9)),
    ),
}


_INF_KEY = 2.0**127
_NAN_KEY = 1.5 * 2.0**127


def _to_key(x):
    y = jnp.clip(x * 0.5, -_INF_KEY, _INF_KEY)
    return jnp.where(x != x, _NAN_KEY, y)


def _from_key(y):
    return jnp.where(y > _INF_KEY, jnp.nan, y + y)


def _ascending(a, b):
    return jnp.minimum(a, b), jnp.maximum(a, b)


def _descending(a, b):
    return jnp.maximum(a, b), jnp.minimum(a, b)


def _bit_clear(d):
    return (lax.broadcasted_iota(jnp.int32, _TILE, 0) & d) == 0


def _roll(x, d):
    return pltpu.roll(x, d % 8, 0)


def _exchange(a, b, d):
    low = _bit_clear(d)
    return jnp.where(low, a, _roll(b, d)), jnp.where(low, _roll(a, -d), b)


def _exchange_all(tiles, d):
    return [t for a, b in zip(tiles[::2], tiles[1::2]) for t in _exchange(a, b, d)]


def _sublane_stage(tiles, d, order):
    out = []
    for a, b in zip(tiles[::2], tiles[1::2]):
        if d == 4:
            low = _bit_clear(4)
            out += order(jnp.where(low, a, b), _roll(jnp.where(low, b, a), 4))
        else:
            out += order(*_exchange(a, b, d))
    return out


def _merge_tiles(a, b, order):
    if not a or not b:
        return list(a) + list(b)
    if len(a) == len(b) == 1:
        return list(order(a[0], b[0]))
    even = _merge_tiles(a[::2], b[::2], order)
    odd = _merge_tiles(a[1::2], b[1::2], order)
    out = [even[0]]
    for o, e in zip(odd, even[1:]):
        out += order(o, e)
    n = min(len(odd), len(even) - 1)
    return out + odd[n:] + even[1 + n :]


def _sort(tiles, bits, order):
    tiles = list(tiles)
    for layer in _NETWORKS[len(tiles)]:
        for i, j in layer:
            tiles[i], tiles[j] = order(tiles[i], tiles[j])
    for done, d in enumerate(bits):
        if done == 0:
            low = _bit_clear(d)
            pairs = list(zip(tiles[::2], tiles[1::2]))
            first = [jnp.where(low, a, _roll(b, d)) for a, b in pairs]
            second = [jnp.where(low, _roll(b, -d), a) for a, b in pairs]
        else:
            tiles = _exchange_all(tiles, d)
            first, second = tiles[::2], [-t for t in tiles[:0:-2]]
        tiles = _merge_tiles(first, second, order)
        for e in bits[: done + 1]:
            tiles = _sublane_stage(tiles, e, order)
    return tiles


def _input_sign(row, bits):
    return jnp.where(((row & bits[1]) == 0) == ((row & bits[2]) == 0), 1.0, -1.0)


def _finish_merge(tiles, order):
    for d in (4, 2, 1):
        tiles = _sublane_stage(tiles, d, order)
    return tiles


def _merge(run, backwards, order, keep):
    return _finish_merge(_merge_tiles(run, backwards[::-1], order)[:keep], order)


def _tiles(x):
    return [x[i : i + 8] for i in range(0, x.shape[0], 8)]


def _one_hot(rows, period, bits=None):
    row = lax.broadcasted_iota(jnp.int32, (rows, 128), 0)
    col = lax.broadcasted_iota(jnp.int32, (rows, 128), 1)
    one = 1.0 if bits is None else _input_sign(row, bits)
    return jnp.where(row == (col & (period - 1)), one, 0.0).astype(jnp.bfloat16)


def _transpose(one_hot, x):
    if x.shape[0] < 128:
        x = jnp.concatenate([x, jnp.zeros((128 - x.shape[0], 128), x.dtype)])
    dims = (((1,), (1,)), ((), ()))
    return lax.dot_general(one_hot, x, dims, preferred_element_type=jnp.float32)


def _pack(tiles):
    words = [lax.bitcast_convert_type(t, jnp.uint32) for t in tiles]
    return [(a >> 16) | b for a, b in zip(words[::2], words[1::2])]


def _as_bf16(words):
    return pltpu.bitcast(words, jnp.bfloat16)


def _as_words(x):
    return pltpu.bitcast(x.astype(jnp.bfloat16), jnp.uint32)


def _in_order(tiles):
    return _tiles(_as_bf16(jnp.concatenate(_pack(tiles))).astype(jnp.float32))


def _sort_kernel(
    x_hbm, out_ref, x_ref, runs, direct, halves, load_sems, send_sems, recv_sems, ready
):
    loads = [
        pltpu.make_async_copy(x_hbm.at[rows], x_ref.at[rows], load_sems.at[i])
        for i, rows in enumerate((pl.ds(0, _LOADED), pl.ds(_LOADED, _DIRECT)))
    ]
    loads[0].start()
    me = lax.axis_index("i")
    barrier = pltpu.get_barrier_semaphore()
    lane = lax.broadcasted_iota(jnp.int32, _TILE, 1)
    low_lanes = lane < 64

    def signal(sem, chip):
        pl.semaphore_signal(
            sem, 1, device_id=(chip,), device_id_type=pl.DeviceIdType.MESH
        )

    def remote(src, dst, send_slot, recv_slot, chip):
        return pltpu.make_async_remote_copy(
            src,
            dst,
            send_sems.at[send_slot],
            recv_sems.at[recv_slot],
            device_id=(chip,),
            device_id_type=pl.DeviceIdType.MESH,
        )

    def run_copy(src, dst):
        return remote(runs.at[src], runs.at[src], dst, src, dst)

    def piece_copy(i):
        if i == 0:
            return remote(x_hbm.at[pl.ds(_LOADED, _DIRECT)], direct, 4, 4, 0)
        rows = pl.ds(8, _LOADED // 2 - 8) if i == 1 else pl.ds(0, 8)
        return remote(halves.at[rows], halves.at[rows], 4 + i, 4 + i, 0)

    def read_run(src):
        words = runs[src]
        words = jnp.concatenate([words, pltpu.roll(words, 64, 1)])
        return _tiles(_as_bf16(words).astype(jnp.float32))

    def write_output(tiles):
        ranks = _as_bf16(jnp.concatenate(_pack(tiles)))
        out_ref[...] = _from_key(_transpose(_one_hot(_COLS, 128), ranks))

    @pl.when(me == 2)
    def _():
        pl.semaphore_wait(barrier, 1)
        piece_copy(0).start()
        signal(ready, 0)
        loads[0].wait()
        keys = _to_key(x_ref[0:_LOADED])
        a, b = keys[0:16], keys[16:32]
        low = lax.broadcasted_iota(jnp.int32, a.shape, 1) < 64
        halves[8:16] = _as_words(jnp.where(low, b, a))
        halves[16:24] = _as_words(jnp.concatenate([keys[_SPLIT:]] * 2))
        piece_copy(1).start()
        halves[0:8] = _as_words(jnp.where(low, a, b))
        piece_copy(2).start()
        loads[1].start()

    @pl.when(me != 2)
    def _():
        loads[1].start()

        @pl.when(me == 0)
        def _():
            for chip in (2, 1, 3):
                signal(barrier, chip)

        @pl.when(me != 0)
        def _():
            signal(barrier, 0)

        loads[0].wait()

    loads[1].wait()
    sign = jnp.where(me % 2 == 0, 1.0, -1.0)
    keys = (_to_key(x_ref[...]) * sign).astype(jnp.bfloat16)
    keys = _transpose(_one_hot(_ROWS, 128, (4, 2, 1)), jnp.concatenate([keys] * 2))
    run = _sort(_tiles(keys), (4, 2, 1), _ascending)
    run = [jnp.where(low_lanes, a, b) * sign for a, b in zip(run[:8], run[8:])]
    runs[me] = jnp.concatenate(_pack(run))

    @pl.when(me % 2 == 1)
    def _():
        pl.semaphore_wait(barrier, 1)
        run_copy(me, 0).start()
        pl.semaphore_wait(ready, 1)
        run_copy(me, 4 - me).start()
        pl.semaphore_wait(ready, 1)
        run_copy(me, 2).start()
        for src in (0, 2, 4 - me):
            run_copy(src, me).wait_recv()
        for dst in (0, 2, 4 - me):
            run_copy(me, dst).wait_send()

    @pl.when(me == 2)
    def _():
        pl.semaphore_wait(barrier, 1)
        for dst in (1, 3):
            run_copy(2, dst).start()
        for i in range(3):
            piece_copy(i).wait_send()
        for dst in (1, 3):
            run_copy(2, dst).wait_send()
        for src in (0, 1, 3):
            run_copy(src, 2).wait_recv()

    @pl.when(me != 0)
    def _():
        r0, r1, r2, r3 = (read_run(src) for src in range(4))
        tiles = _in_order(_merge(r0, r1, _ascending, 32))
        tiles += _in_order(_merge(r3, r2, _descending, 32))
        for upper in (me >= 2, me % 2 == 1):
            n = len(tiles) // 2
            tiles = [
                jnp.where(upper, jnp.maximum(a, b), jnp.minimum(a, b))
                for a, b in zip(tiles[:n], tiles[n:])
            ]
        for d in (8, 4, 2, 1):
            for i in range(16):
                if not i & d:
                    tiles[i], tiles[i + d] = _ascending(tiles[i], tiles[i + d])
        write_output(_finish_merge(tiles, _ascending))

    @pl.when(me == 0)
    def _():
        pl.semaphore_wait(barrier, 2)
        signal(barrier, 2)
        for chip in (1, 3):
            signal(ready, chip)
        for dst in (1, 3):
            run_copy(0, dst).start()
        pl.semaphore_wait(ready, 1)
        for chip in (1, 3):
            signal(ready, chip)
        run_copy(0, 2).start()

        for src in (1, 3):
            run_copy(src, 0).wait_recv()
        low = read_run(0)
        for src in (1, 3):
            low = _in_order(_merge(low, read_run(src), _ascending, 16))
        bits = (1, 4, 2)
        first_one_hot, last_one_hot = _one_hot(128, 128, bits), _one_hot(64, 64, bits)
        for dst in (1, 3, 2):
            run_copy(0, dst).wait_send()

        piece_copy(0).wait_recv()
        keys = _to_key(direct[...])
        piece_copy(1).wait_recv()
        whole = _as_bf16(halves[16 : _LOADED // 2]).astype(jnp.float32)
        whole = jnp.concatenate([whole, keys]).astype(jnp.bfloat16)
        keys = _as_bf16(halves[8:16])
        both = _tiles(_transpose(first_one_hot, jnp.concatenate([keys, keys, whole])))
        first = [jnp.where(lane >> 4 == 1, a, b) for a, b in zip(both[:8], both[8:])]

        piece_copy(2).wait_recv()
        words = halves[0:8]
        words = jnp.concatenate(
            [jnp.where(low_lanes, words, 0), jnp.where(low_lanes, 0, words)]
        )
        last = _tiles(_transpose(last_one_hot, _as_bf16(words)))
        last = [jnp.where(lane < _SPLIT, a, b) for a, b in zip(last, both[:8])]

        run = _exchange_all(_sort(first, bits, _descending), 1)
        low = _in_order(_merge(low, run, _ascending, 16))
        run = _exchange_all(_sort(last, bits, _descending), 1)
        write_output(_merge(low, run, _ascending, 16))


def pallas_dist_sort_i_m128_n64_kernel(x: jax.Array):
    assert x.shape == (_ROWS, _COLS)
    out = pl.pallas_call(
        _sort_kernel,
        out_shape=jax.ShapeDtypeStruct((_COLS, _ROWS), jnp.float32),
        in_specs=[pl.BlockSpec(memory_space=pl.ANY)],
        out_specs=pl.BlockSpec(memory_space=pltpu.VMEM),
        scratch_shapes=[
            pltpu.VMEM((_COLS, _ROWS), jnp.float32),
            pltpu.VMEM((4, 32, 128), jnp.uint32),
            pltpu.VMEM((_DIRECT, _ROWS), jnp.float32),
            pltpu.VMEM((24, 128), jnp.uint32),
            pltpu.SemaphoreType.DMA((2,)),
            pltpu.SemaphoreType.DMA((7,)),
            pltpu.SemaphoreType.DMA((7,)),
            pltpu.SemaphoreType.REGULAR,
        ],
        compiler_params=pltpu.CompilerParams(collective_id=0),
    )(x.T)
    return out.T
```

```python
import jax
import jax.numpy as jnp
from jax import lax
from jax.experimental import pallas as pl
from jax.experimental.pallas import tpu as pltpu

_ROWS, _COLS = 128, 64
_TILE = (8, 128)
_LOADS = ((24, 16), (0, 24), (40, 24))
_LANE_ORDER = (3, 0, 4, 1, 2, 5, 6, 7)

_NETWORK_6 = (
    ((0, 1), (2, 3), (4, 5)),
    ((0, 2), (3, 5), (1, 4)),
    ((0, 1), (2, 3), (4, 5)),
    ((1, 2), (3, 4)),
    ((2, 3),),
)
_NETWORK_16 = (
    ((0, 13), (1, 12), (2, 15), (3, 14), (4, 8), (5, 6), (7, 11), (9, 10)),
    ((0, 5), (1, 7), (2, 9), (3, 4), (6, 13), (8, 14), (10, 15), (11, 12)),
    ((0, 1), (2, 3), (4, 5), (6, 8), (7, 9), (10, 11), (12, 13), (14, 15)),
    ((0, 2), (1, 3), (4, 10), (5, 11), (6, 7), (8, 9), (12, 14), (13, 15)),
    ((1, 2), (3, 12), (4, 6), (5, 7), (8, 10), (9, 11), (13, 14)),
    ((1, 4), (2, 6), (5, 8), (7, 10), (9, 13), (11, 14)),
    ((2, 4), (3, 6), (9, 12), (11, 13)),
    ((3, 5), (6, 8), (7, 9), (10, 12)),
    ((3, 4), (5, 6), (7, 8), (9, 10), (11, 12)),
    ((6, 7), (8, 9)),
)


_INF_KEY = 2.0**127
_NAN_KEY = 1.5 * 2.0**127


def _to_key(x):
    y = jnp.clip(x * 0.5, -_INF_KEY, _INF_KEY)
    return jnp.where(x != x, _NAN_KEY, y)


def _from_key(y):
    return jnp.where(y > _INF_KEY, jnp.nan, y + y)


def _ascending(a, b):
    return jnp.minimum(a, b), jnp.maximum(a, b)


def _descending(a, b):
    return jnp.maximum(a, b), jnp.minimum(a, b)


def _bit_clear(d):
    return (lax.broadcasted_iota(jnp.int32, _TILE, 0) & d) == 0


def _roll(x, d):
    return pltpu.roll(x, d % 8, 0)


def _pairs(tiles):
    return list(zip(tiles[::2], tiles[1::2]))


def _network(tiles, layers, order):
    tiles = list(tiles)
    for layer in layers:
        for i, j in layer:
            tiles[i], tiles[j] = order(tiles[i], tiles[j])
    return tiles


def _exchange(tiles, d):
    low = _bit_clear(d)
    out = []
    for a, b in _pairs(tiles):
        out += [jnp.where(low, a, _roll(b, d)), jnp.where(low, _roll(a, -d), b)]
    return out


def _sublane_stage(tiles, d, order, first=None):
    if d != 4:
        return [t for a, b in _pairs(_exchange(tiles, d)) for t in order(a, b)]
    first = _bit_clear(4) if first is None else first
    out = []
    for a, b in _pairs(tiles):
        out += order(jnp.where(first, a, b), _roll(jnp.where(first, b, a), 4))
    return out


def _merge_tiles(a, b, order):
    if not a or not b:
        return list(a) + list(b)
    if len(a) == len(b) == 1:
        return list(order(a[0], b[0]))
    even = _merge_tiles(a[::2], b[::2], order)
    odd = _merge_tiles(a[1::2], b[1::2], order)
    out = [even[0]]
    for o, e in zip(odd, even[1:]):
        out += order(o, e)
    n = min(len(odd), len(even) - 1)
    return out + odd[n:] + even[1 + n :]


def _finish_merge(tiles, order):
    for d in (4, 2, 1):
        tiles = _sublane_stage(tiles, d, order)
    return tiles


def _merge(run, backwards, order, keep):
    return _finish_merge(_merge_tiles(run, backwards[::-1], order)[:keep], order)


def _merge_sublanes(tiles, order):
    for d in (4, 2):
        low = _bit_clear(d)
        first = [jnp.where(low, a, _roll(b, d)) for a, b in _pairs(tiles)]
        second = [jnp.where(low, _roll(b, -d), a) for a, b in _pairs(tiles)]
        tiles = _merge_tiles(first, second, order)
        if d == 4:
            tiles = _sublane_stage(tiles, 4, order, low == _bit_clear(2))
        else:
            tiles = _sublane_stage(_sublane_stage(tiles, 4, order), 2, order)
    tiles = _exchange(tiles, 1)
    return _merge(tiles[::2], [-t for t in tiles[1::2]], order, len(tiles))


def _tiles(x):
    return [x[i : i + 8] for i in range(0, x.shape[0], 8)]


def _low_lanes(rows):
    return lax.broadcasted_iota(jnp.int32, (rows, 128), 1) < 64


def _one_hot(rows, period, odd_rows=1.0):
    row = lax.broadcasted_iota(jnp.int32, (rows, 128), 0)
    col = lax.broadcasted_iota(jnp.int32, (rows, 128), 1)
    one = jnp.where(row & 1 == 1, odd_rows, 1.0)
    return jnp.where(row == col & (period - 1), one, 0.0).astype(jnp.bfloat16)


def _transpose(one_hot, x):
    if x.shape[0] < 128:
        x = jnp.concatenate([x, jnp.zeros((128 - x.shape[0], 128), x.dtype)])
    dims = (((1,), (1,)), ((), ()))
    return lax.dot_general(one_hot, x, dims, preferred_element_type=jnp.float32)


def _as_bf16(words):
    return pltpu.bitcast(words, jnp.bfloat16)


def _as_words(x):
    return pltpu.bitcast(x, jnp.uint32)


def _pack(paired):
    words = [lax.bitcast_convert_type(t, jnp.uint32) for t in paired]
    return jnp.concatenate([(a >> 16) | b for a, b in _pairs(words)])


def _in_order(words):
    return _tiles(_as_bf16(words).astype(jnp.float32))


def _sort_kernel(
    x_hbm, out_ref, x_ref, runs, direct, pieces, load_sems, send_sems, recv_sems, ready
):
    loads = [
        pltpu.make_async_copy(
            x_hbm.at[pl.ds(*cols)], x_ref.at[pl.ds(*cols)], load_sems.at[i]
        )
        for i, cols in enumerate(_LOADS)
    ]
    me = lax.axis_index("i")
    loads[0].start()
    loads[1].start()
    barrier = pltpu.get_barrier_semaphore()
    odd_chips_in, chip_2_in = ready.at[0], ready.at[1]

    def signal(sem, chip):
        pl.semaphore_signal(
            sem, 1, device_id=(chip,), device_id_type=pl.DeviceIdType.MESH
        )

    def remote(src, dst, send_slot, recv_slot, chip):
        return pltpu.make_async_remote_copy(
            src,
            dst,
            send_sems.at[send_slot],
            recv_sems.at[recv_slot],
            device_id=(chip,),
            device_id_type=pl.DeviceIdType.MESH,
        )

    def run_copy(src, dst):
        return remote(runs.at[src], runs.at[src], dst, src, dst)

    def piece_copy(i):
        if i == 0:
            return remote(x_hbm.at[pl.ds(*_LOADS[2])], direct, 4, 4, 0)
        piece = (pieces.at[0, 0:8], pieces.at[1, 8:20], pieces.at[2, 0:20])[i - 1]
        return remote(piece, piece, 4 + i, 4 + i, 0)

    def read_run(src):
        words = runs[src]
        return _in_order(jnp.concatenate([words, pltpu.roll(words, 64, 1)]))

    def write_output(paired):
        words = _pack(paired)
        bottom = _transpose(_one_hot(_COLS, 128), _as_bf16(words[:32]))
        top = _as_bf16(jnp.concatenate([jnp.zeros_like(words[:32]), words[32:]]))
        top = top[:, :_COLS].T.astype(jnp.float32)
        for i, tile in zip(_LANE_ORDER, _tiles(_from_key(bottom + top))):
            out_ref[8 * i : 8 * i + 8] = tile

    @pl.when(me == 2)
    def _():
        pl.semaphore_wait(barrier, 1)
        signal(chip_2_in, 0)
        piece_copy(0).start()
        low_lanes = _low_lanes(8)

        def half(a, b):
            return _to_key(jnp.where(low_lanes, a, b)).astype(jnp.bfloat16)

        loads[0].wait()
        a, b = _tiles(x_ref[24:40])
        pieces[0, 0:8] = half(a, b)
        piece_copy(1).start()
        pieces[2, 0:8] = half(b, a)
        loads[1].wait()
        a, b, c = _tiles(x_ref[0:24])
        pieces[1, 8:16] = half(a, b)
        pieces[1, 16:24] = half(c, _roll(c, 4))
        piece_copy(2).start()
        pieces[2, 8:16] = half(b, a)
        pieces[2, 16:24] = half(_roll(c, 4), c)
        piece_copy(3).start()
        loads[2].start()

    @pl.when(me != 2)
    def _():
        loads[2].start()

        @pl.when(me == 0)
        def _():
            for chip in (2, 1, 3):
                signal(barrier, chip)

        @pl.when(me != 0)
        def _():
            signal(barrier, 0)

        loads[0].wait()
        loads[1].wait()

    loads[2].wait()
    sign = jnp.where(me % 2 == 0, 1.0, -1.0)
    keys = jnp.concatenate([x_ref[8 * i : 8 * i + 8] for i in _LANE_ORDER])
    keys = (_to_key(keys) * sign).astype(jnp.bfloat16)
    keys = _transpose(_one_hot(_ROWS, 128, -1.0), jnp.concatenate([keys, keys]))
    run = _network(_tiles(keys), _NETWORK_16, _ascending)
    run = _merge_sublanes(run, _ascending)
    runs[me] = _pack(
        [jnp.where(_low_lanes(8), a, b) * sign for a, b in zip(run[:8], run[8:])]
    )

    for chip in (1, 3):

        @pl.when(me == chip)
        def _():
            pl.semaphore_wait(barrier, 1)
            run_copy(chip, 0).start()
            pl.semaphore_wait(odd_chips_in, 1)
            run_copy(chip, 4 - chip).start()
            pl.semaphore_wait(chip_2_in, 1)
            run_copy(chip, 2).start()
            for other in (0, 2, 4 - chip):
                run_copy(chip, other).wait_send()
                run_copy(other, chip).wait_recv()

    @pl.when(me == 2)
    def _():
        pl.semaphore_wait(barrier, 1)
        for dst in (1, 3):
            run_copy(2, dst).start()
        for i in range(4):
            piece_copy(i).wait_send()
        for dst in (1, 3):
            run_copy(2, dst).wait_send()
        for src in (0, 1, 3):
            run_copy(src, 2).wait_recv()

    @pl.when(me != 0)
    def _():
        r0, r1, r2, r3 = (read_run(src) for src in range(4))
        tiles = _in_order(_pack(_merge(r0, r1, _ascending, 32)))
        tiles += _in_order(_pack(_merge(r3, r2, _descending, 32)))
        for upper in (me >= 2, me % 2 == 1):
            n = len(tiles) // 2
            tiles = [
                jnp.where(upper, jnp.maximum(a, b), jnp.minimum(a, b))
                for a, b in zip(tiles[:n], tiles[n:])
            ]
        stages = [[(i, i + d) for i in range(16) if not i & d] for d in (8, 4, 2, 1)]
        write_output(_finish_merge(_network(tiles, stages, _ascending), _ascending))

    @pl.when(me == 0)
    def _():
        pl.semaphore_wait(barrier, 2)
        signal(barrier, 2)
        for chip in (1, 3):
            signal(odd_chips_in, chip)
        for dst in (1, 3):
            run_copy(0, dst).start()
        pl.semaphore_wait(chip_2_in, 1)
        for chip in (1, 3):
            signal(chip_2_in, chip)
        run_copy(0, 2).start()

        def keep_lowest(low, backwards):
            return _merge(low, backwards, _ascending, 16)

        for src in (1, 3):
            run_copy(src, 0).wait_recv()
        low = read_run(0)
        for src in (1, 3):
            low = _in_order(_pack(keep_lowest(low, read_run(src))))
        one_hot = _one_hot(64, 64, -1.0)
        for dst in (1, 3):
            run_copy(0, dst).wait_send()

        piece_copy(0).wait_recv()
        keys = _to_key(direct[...])
        whole = _as_words(jnp.concatenate([keys[:8], keys]).astype(jnp.bfloat16))
        whole = [jnp.where(_low_lanes(16), *pair) for pair in ((whole, 0), (0, whole))]
        piece_copy(1).wait_recv()
        run_copy(0, 2).wait_send()

        def read_half(h):
            piece_copy(2 + h).wait_recv()
            if h == 0:
                head = jnp.concatenate([pieces[0, 0:8], pieces[1, 8:16]])
            else:
                head = pieces[2, 0:16]
            words = []
            for rows in (head, pieces[1 + h, 16:20]):
                rows = _as_words(rows)
                for pair in ((rows, 0), (0, rows))[:: 1 - 2 * h]:
                    words.append(jnp.where(_low_lanes(rows.shape[0]), *pair))
            words.append(whole[h][4:])
            return _transpose(one_hot, _as_bf16(jnp.concatenate(words)))

        def start_sort(half):
            tiles = _tiles(half)
            early = [tiles[i] for i in (0, 2, 4, 6, 1, 3)]
            return _network(early, _NETWORK_6, _descending), _descending(*tiles[5::2])

        def end_sort(early, late):
            run = _merge_tiles(early, late, _descending)
            return _in_order(_pack(_merge_sublanes(run, _descending)))

        @pl.when(me < 1)
        def _():
            x_ref[...] = read_half(0)

        last = start_sort(read_half(1))
        low = _in_order(_pack(keep_lowest(low, end_sort(*start_sort(x_ref[...])))))

        @pl.when(me < 1)
        def _():
            write_output(keep_lowest(low, end_sort(*last)))


def pallas_dist_sort_i_m128_n64_kernel(x: jax.Array):
    assert x.shape == (_ROWS, _COLS)
    out = pl.pallas_call(
        _sort_kernel,
        out_shape=jax.ShapeDtypeStruct((_COLS, _ROWS), jnp.float32),
        in_specs=[pl.BlockSpec(memory_space=pl.ANY)],
        out_specs=pl.BlockSpec(memory_space=pltpu.VMEM),
        scratch_shapes=[
            pltpu.VMEM((_COLS, _ROWS), jnp.float32),
            pltpu.VMEM((4, 32, 128), jnp.uint32),
            pltpu.VMEM((24, _ROWS), jnp.float32),
            pltpu.VMEM((3, 32, 128), jnp.bfloat16),
            pltpu.SemaphoreType.DMA((3,)),
            pltpu.SemaphoreType.DMA((8,)),
            pltpu.SemaphoreType.DMA((8,)),
            pltpu.SemaphoreType.REGULAR((2,)),
        ],
        compiler_params=pltpu.CompilerParams(
            collective_id=0, disable_bounds_checks=True, disable_semaphore_checks=True
        ),
    )(x.T)
    return out.T
```
